```python
import numpy as np

kernel_name = "dist_sparse_attn_blocksparse_kvseq_b2_sq256_skv256_hq4_dh64"

def setup_inputs():
    x = np.random.randn(2, 256, 512).astype(np.float32)
    Wq = np.random.randn(512, 256).astype(np.float32) * 0.02
    K_ext = np.random.randn(2, 1024, 4, 64).astype(np.float32)
    V_ext = np.random.randn(2, 1024, 4, 64).astype(np.float32)
    Wo = np.random.randn(256, 512).astype(np.float32) * 0.02
    return {"x": x, "Wq": Wq, "K_ext": K_ext, "V_ext": V_ext, "Wo": Wo}

def reference(x, Wq, K_ext, V_ext, Wo):
    B, Sq, Skv, Hq, Dh = 2, 256, 1024, 4, 64
    Q = (x @ Wq).reshape(B, Sq, Hq, Dh)
    qb = (np.arange(Sq) // 64)[:, None]
    kb = (np.arange(Skv) // 64)[None, :]
    mask = (qb == kb) | (kb == 0) | ((qb + kb) % 3 == 0)
    scores = np.einsum('bihd,bjhd->bhij', Q, K_ext).astype(np.float32) * 0.125
    scores = np.where(mask[None, None, :, :], scores, -1e9)
    scores_max = scores.max(axis=-1, keepdims=True)
    w = np.exp(scores - scores_max)
    row_keep = mask.any(axis=1)
    w_sum = np.where(row_keep[None, None, :, None], w.sum(axis=-1, keepdims=True), 1.0)
    w = w / w_sum
    w = np.where(row_keep[None, None, :, None], w, 0.0)
    ctx = np.einsum('bhij,bjhd->bihd', w, V_ext).reshape(B, Sq, Hq * Dh)
    return ctx @ Wo
```

```python
import functools
import math

import jax
import jax.numpy as jnp
from jax import lax
from jax.experimental import pallas as pl
from jax.experimental.pallas import tpu as pltpu

B, SQ, DM, H, DH = 2, 256, 512, 4, 64
HD = H * DH
SKV = 256
QSCALE = 0.125 * math.log2(math.e)
NEG = -1e30
TA, TB = 0, 1
TILE_QB = ((0, 3), (1, 2))
A_, B_, C_, D_ = 0, 1, 2, 3
ALL, P0, P1 = (0, 1, 2, 3), (0, 1), (2, 3)
NS = (4, 2)
N_LOAD, N_SEND, N_RECV = 17, 40, 38
bf16, f32, i32 = jnp.bfloat16, jnp.float32, jnp.int32
MESH = pl.DeviceIdType.MESH
NT = (((1,), (1,)), ((), ()))
TN = (((0,), (0,)), ((), ()))
TT = (((0,), (1,)), ((), ()))


def _pack(v):
    return pltpu.bitcast(v.astype(bf16), i32)


def _unpack(v):
    return pltpu.bitcast(v, bf16)


def _cat(parts):
    return parts[0] if len(parts) == 1 else jnp.concatenate(parts, axis=0)


def _kernel(x_hbm, wq_hbm, kt_hbm, vt_hbm, wo_hbm, out_ref,
            x_v, wq_v, kt_v, vt_v, wo_v, wq_b, wo_b,
            kvs, kvr, s1s, s1r, s2s, s2r, ctx, qs, qr, krow,
            lsem, ssem, rsem, csem):
    me = lax.axis_index("i")
    bar = pltpu.get_barrier_semaphore()
    lo128 = lax.broadcasted_iota(i32, (128, 128), 1) < 64
    lo64 = lax.broadcasted_iota(i32, (64, 128), 1) < 64
    lo32 = lax.broadcasted_iota(i32, (32, 128), 1) < 64

    sem_ids = [{} for _ in range(4)]

    def recv_sem(dev, key):
        return rsem.at[sem_ids[dev].setdefault(key, len(sem_ids[dev]))]

    def chip_program(chip):
        loads, sends, qv, pend, own, krows = {}, [], {}, {}, {}, set()
        n_issued, n_drained = [0], [0]

        def load(name, pairs):
            cps = [pltpu.make_async_copy(s, d, lsem.at[n_issued[0]]) for s, d in pairs]
            for cp in cps:
                cp.start()
            n_issued[0] += 1
            loads[name] = cps

        def wait_load(*names):
            for name in names:
                for cp in loads.pop(name):
                    cp.wait()

        def ld_x(b, t):
            rows = [(64, 192)] if t == TB else [(0, 64), (192, 256)]
            load(("x", b, t), [(x_hbm.at[b, r0:r1], x_v.at[b, r0:r1]) for r0, r1 in rows])

        def ld_wq(p):
            load(("wq", p), [(wq_hbm.at[:, p * 128:(p + 1) * 128], wq_v.at[:, p * 128:(p + 1) * 128])])

        def ld_kv(name, which, b, ps, ts):
            r0, r1 = ps[0] * 128, (ps[-1] + 1) * 128
            c0, c1 = ts[0] * 128, (ts[-1] + 1) * 128
            refs = {"k": (kt_hbm, kt_v), "v": (vt_hbm, vt_v)}
            load(name, [(refs[w][0].at[b, r0:r1, c0:c1], refs[w][1].at[b, r0:r1, c0:c1]) for w in which])

        def ld_wo():
            load("wo", [(wo_hbm, wo_v)])

        def prep_wq(p):
            wait_load(("wq", p))
            wq_b[:, p * 128:(p + 1) * 128] = _pack(wq_v[:, p * 128:(p + 1) * 128] * QSCALE)

        def prep_wo():
            wait_load("wo")
            wo_b[...] = _pack(wo_v[...])

        def send(src, dst, key, dev):
            cp = pltpu.make_async_remote_copy(
                src_ref=src, dst_ref=dst, send_sem=ssem.at[len(sends)], recv_sem=recv_sem(dev, key),
                device_id=(dev,), device_id_type=MESH)
            cp.start()
            sends.append(cp)

        def recv(dst, key):
            pltpu.make_async_remote_copy(
                src_ref=dst, dst_ref=dst, send_sem=ssem.at[0], recv_sem=recv_sem(chip, key),
                device_id=(chip,), device_id_type=MESH).wait_recv()

        def drain(keep=0):
            while n_drained[0] < len(sends) - keep:
                sends[n_drained[0]].wait_send()
                n_drained[0] += 1

        def signal(sem, dev):
            pl.semaphore_signal(sem, inc=1, device_id=(dev,), device_id_type=MESH)

        def qproj(b, t, ps):
            xs = x_v[b, 64:192, :] if t == TB else _cat([x_v[b, 0:64, :], x_v[b, 192:256, :]])
            w = _unpack(wq_b[:, ps[0] * 128:(ps[-1] + 1) * 128])
            q = jnp.dot(xs.astype(bf16), w, preferred_element_type=f32)
            for i, p in enumerate(ps):
                qv[b, t, p] = q[:, i * 128:(i + 1) * 128]

        def kt_tile(b, p, c0, c1):
            return kt_v[b, p * 128:(p + 1) * 128, c0:c1]

        def vt_tile(b, h, c0, c1):
            return vt_v[b, h * 64:(h + 1) * 64, c0:c1]

        def vt_pair(b, p, c0, c1):
            return vt_v[b, p * 128:(p + 1) * 128, c0:c1]

        def k03(b, p):
            return jnp.where(lo128, kt_tile(b, p, 0, 128), kt_tile(b, p, 128, 256))

        def k21(b, p):
            return jnp.where(lo128, kt_tile(b, p, 128, 256), kt_tile(b, p, 0, 128))

        def plain(p):
            return p

        def upper(p):
            return _cat([jnp.zeros_like(p), p])

        def lower(p):
            return _cat([p, jnp.zeros_like(p)])

        def lohi(p):
            return _cat([jnp.where(lo64, p, 0.0), jnp.where(lo64, 0.0, p)])

        def hilo(p):
            return _cat([jnp.where(lo64, 0.0, p), jnp.where(lo64, p, 0.0)])

        def unit_scores(b, t, h, extra):
            p, e = h // 2, h % 2
            if (b, t, p) in qv:
                q = qv[b, t, p]
                w = (jnp.where(lo128, q, 0.0) if e == 0 else jnp.where(lo128, 0.0, q)).astype(bf16)
            else:
                w = _unpack(jnp.where(lo64, qr[p], 0) if e == 0 else jnp.where(lo64, 0, qr[p]))

            def qk_t(kt):
                return lax.dot_general(kt.astype(bf16), w, TT, preferred_element_type=f32)

            def qk_r(k):
                return lax.dot_general(_unpack(k), w, NT, preferred_element_type=f32)

            def vt(c0, c1):
                return lambda: vt_tile(b, h, c0, c1).astype(bf16)

            def vsel(ca, cb):
                return lambda: jnp.where(
                    lo64, vt_tile(b, h, ca, ca + 128), vt_tile(b, h, cb, cb + 128)).astype(bf16)

            if t == TA and chip in (A_, D_):
                terms = [(qk_t(k03(b, p)), vsel(0, 128), plain)]
            elif t == TA and chip == B_:
                terms = [(qk_t(kt_tile(b, p, 128, 192)), vt(128, 192), plain)]
            elif chip == A_:
                terms = [(qk_t(kt_tile(b, p, 0, 128)), vt(0, 128), plain),
                         (qk_t(kt_tile(b, p, 128, 192)), vt(128, 192), plain)]
            elif chip == B_:
                s0 = qk_t(kt_tile(b, p, 0, 128))
                s1 = qk_t(kt_tile(b, p, 128, 256))
                terms = [(jnp.where(lo64, s0[64:128], s0[0:64]), vt(0, 128), hilo),
                         (jnp.where(lo64, NEG, s1[64:128]), vt(128, 256), upper)]
            elif chip == C_:
                s1 = qk_r(krow[b, p, 0:64]) if (b, p) in krows else qk_t(kt_tile(b, p, 128, 256))
                s0 = qk_r(krow[b, p, 64:96])
                terms = [(jnp.where(lo64, s1[64:128], s1[0:64]), vt(128, 256), hilo),
                         (jnp.where(lo64, s0, NEG), vt(0, 64), plain)]
            else:
                if (b, p) in krows:
                    sa, sb = qk_r(krow[b, p, 0:32]), qk_r(krow[b, p, 32:64])
                else:
                    s0 = qk_t(k21(b, p))
                    sa, sb = s0[0:64], s0[64:128]
                terms = [(jnp.where(lo64, sa, sb), vsel(128, 0), lohi)]

            if extra == "fromC":
                terms.append((qk_r(kvr[p, 32:64]), lambda: _unpack(kvr[p, 0:32]), upper if e else lower))
            elif extra == "fromB":
                terms.append((qk_t(_unpack(kvr[p])[:, 0:64]),
                              lambda: _unpack(kvr[p, e * 32:(e + 1) * 32]), upper))
            elif extra == "fromD":
                terms.append((qk_t(_unpack(kvr[2 + 2 * p])),
                              lambda: _unpack(kvr[3 + 2 * p, e * 32:(e + 1) * 32]), plain))
            return terms

        def qks(*groups):
            units = [(b, t, h, extra) for b, t, hs, extra in groups for h in hs]
            scored = [unit_scores(*u) for u in units]
            for (b, t, h, _), terms in zip(units, scored):
                m = functools.reduce(jnp.maximum, [jnp.max(s, axis=0, keepdims=True) for s, _, _ in terms])
                ps = [jnp.exp2(s - m) for s, _, _ in terms]
                l = functools.reduce(jnp.add, [jnp.sum(p, axis=0, keepdims=True) for p in ps])
                pend[b, t, h] = ([(vget, lay(p).astype(bf16)) for p, (_, vget, lay) in zip(ps, terms)], m, l)

        def pvs(*groups):
            for b, t, hs in groups:
                for h in hs:
                    pw, m, l = pend.pop((b, t, h))
                    o = functools.reduce(
                        jnp.add, [jnp.dot(vget(), w, preferred_element_type=f32) for vget, w in pw])
                    own[b, t, h] = (o, m, l)

        def put(ref, part):
            o, m, l = part
            ref[0:32, :] = _pack(o)
            ref[32:33, :] = lax.bitcast_convert_type(m, i32)
            ref[33:34, :] = lax.bitcast_convert_type(l, i32)

        def stats(ref):
            return (lax.bitcast_convert_type(ref[32:33, :], f32), lax.bitcast_convert_type(ref[33:34, :], f32))

        def weights(ma, la, mb, lb, final):
            m = jnp.maximum(ma, mb)
            ca, cb = jnp.exp2(ma - m), jnp.exp2(mb - m)
            l = ca * la + cb * lb
            if final:
                inv = 1.0 / l
                ca, cb = ca * inv, cb * inv
            return ca, cb, m, l

        def merge(part, ref, final=False):
            oa, ma, la = part
            ca, cb, m, l = weights(ma, la, *stats(ref), final)
            return ca * oa + cb * _unpack(ref[0:32, :]).astype(f32), m, l

        def pieces(n):
            r = 32 // n
            return [(32 - (j + 1) * r, 32 - j * r) for j in range(n)]

        def put_s1(b, hs):
            for h in hs:
                put(s1s.at[b * 4 + h], own.pop((b, TB, h)))

        def send_s1(b, hs, dev):
            for h in hs:
                send(s1s.at[b * 4 + h], s1r.at[b * 4 + h], ("s1", b, h), dev)

        def recv_s1(b, hs):
            for h in hs:
                recv(s1r.at[b * 4 + h], ("s1", b, h))

        def xchg(items, n=1):
            for b, t, h, _ in items:
                if t == TB:
                    own[b, t, h] = merge(own[b, t, h], s1r.at[b * 4 + h])
                put(s2s.at[t * 8 + b * 4 + h], own[b, t, h])
            for b, t, h, dev in items:
                u = t * 8 + b * 4 + h
                for j, (r0, r1) in enumerate(pieces(n)):
                    r1 = 34 if j == 0 else r1
                    send(s2s.at[u, r0:r1], s2r.at[u, r0:r1], ("s2", u, j), dev)

        def fin(b, t, h, dev, n=1):
            u = t * 8 + b * 4 + h
            oa, ma, la = own.pop((b, t, h))
            for j, (r0, r1) in enumerate(pieces(n)):
                recv(s2r.at[u, r0:(34 if j == 0 else r1)], ("s2", u, j))
                if j == 0:
                    ca, cb, _, _ = weights(ma, la, *stats(s2r.at[u]), True)
                    oa = oa * ca
                o = oa[2 * r0:2 * r1] + cb * _unpack(s2r[u, r0:r1, :]).astype(f32)
                ctx[b, t, h * 32 + r0:h * 32 + r1, :] = _pack(o)
                rows = ctx.at[b, t, h * 32 + r0:h * 32 + r1]
                send(rows, rows, ("f", u, j), dev)

        def recv_f(b, t, hs, n=1):
            for h in hs:
                for j, (r0, r1) in enumerate(pieces(n)):
                    recv(ctx.at[b, t, h * 32 + r0:h * 32 + r1], ("f", t * 8 + b * 4 + h, j))

        def oproj(tiles, hs=ALL, acc=False):
            for b, t in tiles:
                if hs == ALL:
                    c, w = ctx[b, t], wo_b[...]
                else:
                    c = _cat([ctx[b, t, h * 32:(h + 1) * 32, :] for h in hs])
                    w = _cat([wo_b[h * 32:(h + 1) * 32, :] for h in hs])
                o = lax.dot_general(_unpack(c), _unpack(w), TN, preferred_element_type=f32)
                for i, qb in enumerate(TILE_QB[t]):
                    if acc:
                        out_ref[b, qb * 64:(qb + 1) * 64, :] += o[i * 64:(i + 1) * 64]
                    else:
                        out_ref[b, qb * 64:(qb + 1) * 64, :] = o[i * 64:(i + 1) * 64]

        if chip == A_:
            signal(bar, B_)
            signal(bar, D_)
            ld_wq(0); ld_wq(1); ld_x(0, TA); ld_x(1, TA); ld_x(1, TB)
            ld_kv("k1", "k", 1, (0, 1), (0, 1)); ld_kv("v1", "v", 1, (0, 1), (0, 1))
            ld_x(0, TB)
            ld_kv("k0", "k", 0, (0, 1), (0, 1)); ld_kv("v0", "v", 0, (0, 1), (0, 1))
            ld_wo()
            prep_wq(0); prep_wq(1)
            for b in range(2):
                wait_load(("x", b, TA)); qproj(b, TA, (0, 1))
                for p in range(2):
                    qs[b * 2 + p] = _pack(qv[b, TA, p])
            pl.semaphore_wait(bar, 2)
            for b, p in ((0, 0), (1, 1), (0, 1), (1, 0)):
                send(qs.at[b * 2 + p], qr.at[p], ("q", p), D_ if b == 0 else B_)
            for b in (1, 0):
                wait_load(("x", b, TB)); qproj(b, TB, (0, 1))
                wait_load(f"k{b}"); qks((b, TB, ALL, None))
                wait_load(f"v{b}"); pvs((b, TB, ALL))
                put_s1(b, ALL)
                send_s1(b, P0, B_); send_s1(b, P1, D_)
            for s in (0, 2, 4):
                recv(kvr.at[s], ("kv", s))
            qks((0, TA, P0, "fromB"), (1, TA, ALL, "fromD"))
            pvs((0, TA, P0))
            xchg([(0, TA, h, D_) for h in P0])
            prep_wo()
            recv(kvr.at[3], ("kv", 3)); recv(kvr.at[1], ("kv", 1))
            pvs((1, TA, P0))
            qks((0, TA, P1, "fromB"))
            xchg([(1, TA, h, B_) for h in P0])
            pvs((0, TA, P1))
            xchg([(0, TA, h, D_) for h in P1])
            recv(kvr.at[5], ("kv", 5))
            pvs((1, TA, P1))
            xchg([(1, TA, h, B_) for h in P1])
            for i in range(4):
                fin(1, TA, (2, 3, 0, 1)[i], D_)
                fin(0, TA, i, B_)
            oproj([(1, TA), (0, TA)])
            drain(4)
            recv_f(1, TB, (0, 2, 1, 3), NS[1])
            oproj([(1, TB)])
            drain()
            recv_f(0, TB, (0, 2), NS[0])
            oproj([(0, TB)], (0, 2))
            recv_f(0, TB, (1, 3), NS[0])
            oproj([(0, TB)], (1, 3), acc=True)

        elif chip == C_:
            ships = (((0, 0), (1, 1)), ((0, 1), (1, 0)))
            for grp in ships:
                for w in "kv":
                    for b, p in grp:
                        ld_kv(("T0", w, b, p), w, b, (p,), (0,))
            ld_wq(0); ld_wq(1); ld_x(1, TB)
            ld_kv("k1", "k", 1, (0, 1), (1,)); ld_kv("v1", "v", 1, (0, 1), (1,))
            ld_x(0, TB)
            ld_kv("k0", "k", 0, (0, 1), (1,)); ld_kv("v0", "v", 0, (0, 1), (1,))
            ld_wo()
            pl.semaphore_wait(bar, 2)
            signal(csem, B_)
            signal(csem, D_)
            for grp in ships:
                wait_load(*[("T0", "k", b, p) for b, p in grp])
                for b, p in grp:
                    kr = kt_tile(b, p, 0, 128).T
                    kvs[b * 2 + p, 32:64, :] = _pack(kr[64:128])
                    krow[b, p, 64:96, :] = _pack(kr[0:64])
                for b, p in grp:
                    send(kvs.at[b * 2 + p, 32:64], kvr.at[p, 32:64], ("k", p), D_ if b == 0 else B_)
                wait_load(*[("T0", "v", b, p) for b, p in grp])
                for b, p in grp:
                    kvs[b * 2 + p, 0:32, :] = jnp.where(
                        lo32, pltpu.roll(_pack(vt_tile(b, 2 * p, 0, 128)), 64, 1),
                        _pack(vt_tile(b, 2 * p + 1, 0, 128)))
                for b, p in grp:
                    send(kvs.at[b * 2 + p, 0:32], kvr.at[p, 0:32], ("v", p), D_ if b == 0 else B_)
            prep_wq(0); prep_wq(1)
            wait_load(("x", 1, TB)); qproj(1, TB, (0, 1))
            wait_load("k1", "v1")
            qks((1, TB, ALL, None)); pvs((1, TB, ALL))
            recv_s1(1, (2,)); xchg([(1, TB, 2, D_)], NS[1])
            recv_s1(1, (0,)); xchg([(1, TB, 0, B_)], NS[1])
            wait_load(("x", 0, TB), "k0")
            qproj(0, TB, (0, 1))
            for p in range(2):
                krow[0, p, 0:64, :] = _pack(kt_tile(0, p, 128, 256).T)
                krows.add((0, p))
            recv_s1(1, (3, 1))
            xchg([(1, TB, 1, B_), (1, TB, 3, D_)], NS[1])
            wait_load("v0")
            qks((0, TB, (0, 2, 1, 3), None))
            pvs((0, TB, (0, 2)))
            recv_s1(0, (2, 0))
            xchg([(0, TB, 0, B_), (0, TB, 2, D_)], NS[0])
            pvs((0, TB, (1, 3)))
            recv_s1(0, (1,)); xchg([(0, TB, 1, B_)], NS[0])
            recv_s1(0, (3,)); xchg([(0, TB, 3, D_)], NS[0])
            prep_wo()
            for b in (1, 0):
                for e in range(2):
                    fin(b, TB, e, D_)
                    fin(b, TB, 2 + e, B_)
            oproj([(1, TB), (0, TB)])
            recv_f(0, TA, P0); recv_f(1, TA, P0)
            oproj([(0, TA), (1, TA)], P0)
            drain()
            recv_f(0, TA, P1); recv_f(1, TA, P1)
            oproj([(0, TA), (1, TA)], P1, acc=True)

        else:
            pg, pk, ba = (0, 1, 0) if chip == D_ else (1, 0, 1)
            HG, HK = (P0, P1)[pg], (P0, P1)[pk]
            signal(bar, A_)
            signal(bar, C_)
            if chip == D_:
                ld_kv("k10", "k", 1, (0,), (0, 1)); ld_kv("k11", "k", 1, (1,), (0, 1))
                ld_wq(0); ld_x(1, TB)
                ld_kv("v10", "v", 1, (0,), (0, 1))
                ld_x(0, TB)
                ld_kv("k00", "k", 0, (0,), (0, 1))
                ld_kv("v11", "v", 1, (1,), (0, 1))
                ld_kv("v00", "v", 0, (0,), (0, 1))
                ld_wq(1)
                ld_kv("k01", "k", 0, (1,), (0, 1)); ld_kv("v01", "v", 0, (1,), (0, 1))
                rest = ("k01", "v01")
                ld_wo()
                pl.semaphore_wait(bar, 1)

                def ship(w, p):
                    wait_load(f"{w}1{p}")
                    s = 2 * p + (w == "v")
                    kvs[s] = _pack(k03(1, p) if w == "k" else
                                   jnp.where(lo128, vt_pair(1, p, 0, 128), vt_pair(1, p, 128, 256)))
                    send(kvs.at[s], kvr.at[2 + s], ("kv", 2 + s), A_)

                ship("k", 0); ship("k", 1)
                krow[1, 0, 0:64, :] = _pack(k21(1, 0).T)
                krows.add((1, 0))
                prep_wq(0)
                pl.semaphore_wait(csem, 1)
                wait_load(("x", 1, TB)); qproj(1, TB, (0,))
                qks((1, TB, HG, None))
                ship("v", 0)
                pvs((1, TB, HG))
                put_s1(1, HG); send_s1(1, HG, C_)
                wait_load(("x", 0, TB)); qproj(0, TB, (0,))
                wait_load("k00"); qks((0, TB, HG, None))
                ship("v", 1)
                wait_load("v00"); pvs((0, TB, HG))
            else:
                ld_kv("T1_0", "kv", 0, (0,), (1,))
                ld_wq(1); ld_x(1, TB)
                ld_kv("k11", "k", 1, (1,), (0, 1)); ld_kv("v11", "v", 1, (1,), (0, 1))
                ld_kv("T1_1", "kv", 0, (1,), (1,))
                ld_x(0, TB)
                ld_kv("T0_1", "kv", 0, (1,), (0,))
                ld_wq(0)
                ld_kv("k10", "k", 1, (0,), (0, 1)); ld_kv("v10", "v", 1, (0,), (0, 1))
                ld_kv("T0_0", "kv", 0, (0,), (0,))
                rest = ("k10", "v10", "T0_0")
                ld_wo()
                pl.semaphore_wait(bar, 1)

                def ship(p):
                    wait_load(f"T1_{p}")
                    kvs[p] = jnp.where(lo64, _pack(kt_tile(0, p, 128, 256)),
                                       pltpu.roll(_pack(vt_pair(0, p, 128, 256)), 64, 1))
                    send(kvs.at[p], kvr.at[p], ("kv", p), A_)

                ship(0)
                prep_wq(1)
                wait_load(("x", 1, TB)); qproj(1, TB, (1,))
                wait_load("k11"); qks((1, TB, HG, None))
                wait_load("v11"); pvs((1, TB, HG))
                put_s1(1, HG)
                pl.semaphore_wait(csem, 1)
                send_s1(1, HG, C_)
                ship(1)
                wait_load(("x", 0, TB)); qproj(0, TB, (1,))
                wait_load("T0_1")
                qks((0, TB, HG, None)); pvs((0, TB, HG))
            put_s1(0, HG); send_s1(0, HG, C_)
            recv(qr.at[pg], ("q", pg)); recv(kvr.at[pg, 32:64], ("k", pg))
            qks((ba, TA, HG, "fromC"))
            recv(kvr.at[pg, 0:32], ("v", pg))
            pvs((ba, TA, HG))
            xchg([(ba, TA, h, A_) for h in HG])
            prep_wq(pk)
            wait_load(*rest)
            recv(qr.at[pk], ("q", pk)); recv(kvr.at[pk, 32:64], ("k", pk))
            qks((ba, TA, HK, "fromC"))
            qproj(1, TB, (pk,)); qproj(0, TB, (pk,))
            recv(kvr.at[pk, 0:32], ("v", pk))
            pvs((ba, TA, HK))
            qks((1, TB, HK, None), (0, TB, HK, None))
            xchg([(ba, TA, h, A_) for h in HK])
            pvs((1, TB, HK), (0, TB, HK))
            recv_s1(1, HK); xchg([(1, TB, h, C_) for h in HK])
            prep_wo()
            for h in HK:
                recv_s1(0, (h,)); xchg([(0, TB, h, C_)])
            fin(1, TB, HK[0], A_, NS[1])
            fin(1, TB, HK[1], A_, NS[1])
            if chip == D_:
                fin(ba, TA, 0, C_)
            fin(0, TB, HK[0], A_, NS[0])
            if chip == B_:
                fin(ba, TA, 0, C_)
            fin(0, TB, HK[1], A_, NS[0])
            for h in (1, 2, 3):
                fin(ba, TA, h, C_)
            oproj([(ba, TA)])
            oproj([(1, TB), (0, TB)], HK)
            recv_f(1 - ba, TA, HK)
            oproj([(1 - ba, TA)], HK)
            last = [(1 - ba, TA), (1, TB)] if chip == D_ else [(1, TB), (1 - ba, TA)]
            for b, t in last:
                recv_f(b, t, HG)
            oproj(last, HG, acc=True)
            drain()
            recv_f(0, TB, HG)
            oproj([(0, TB)], HG, acc=True)

        assert not loads and not own and not pend
        assert n_issued[0] <= N_LOAD and n_drained[0] == len(sends) <= N_SEND

    for chip in range(4):
        pl.when(me == chip)(functools.partial(chip_program, chip))
    assert max(len(ids) for ids in sem_ids) <= N_RECV


def pallas_dist_sparse_attn_blocksparse_kvseq_b2_sq256_skv256_hq4_dh64_kernel(
    x: jax.Array,
    Wq: jax.Array,
    K_ext: jax.Array,
    V_ext: jax.Array,
    Wo: jax.Array,
):
    kt = jnp.transpose(K_ext, (0, 2, 3, 1)).reshape(B, HD, SKV)
    vt = jnp.transpose(V_ext, (0, 2, 3, 1)).reshape(B, HD, SKV)
    return pl.pallas_call(
        _kernel,
        out_shape=jax.ShapeDtypeStruct((B, SQ, DM), f32),
        in_specs=[pl.BlockSpec(memory_space=pl.ANY)] * 5,
        out_specs=pl.BlockSpec(memory_space=pltpu.VMEM),
        scratch_shapes=[
            pltpu.VMEM((B, SQ, DM), f32),
            pltpu.VMEM((DM, HD), f32),
            pltpu.VMEM((B, HD, SKV), f32),
            pltpu.VMEM((B, HD, SKV), f32),
            pltpu.VMEM((HD, DM), f32),
            pltpu.VMEM((DM // 2, HD), i32),
            pltpu.VMEM((HD // 2, DM), i32),
            pltpu.VMEM((4, 64, 128), i32),
            pltpu.VMEM((6, 64, 128), i32),
            pltpu.VMEM((8, 34, 128), i32),
            pltpu.VMEM((8, 34, 128), i32),
            pltpu.VMEM((16, 34, 128), i32),
            pltpu.VMEM((16, 34, 128), i32),
            pltpu.VMEM((B, 2, 128, 128), i32),
            pltpu.VMEM((4, 64, 128), i32),
            pltpu.VMEM((2, 64, 128), i32),
            pltpu.VMEM((2, 2, 96, 128), i32),
            pltpu.SemaphoreType.DMA((N_LOAD,)),
            pltpu.SemaphoreType.DMA((N_SEND,)),
            pltpu.SemaphoreType.DMA((N_RECV,)),
            pltpu.SemaphoreType.REGULAR,
        ],
        compiler_params=pltpu.CompilerParams(collective_id=0, disable_semaphore_checks=True),
    )(x, Wq, kt, vt, Wo)
```
